```python
import numpy as np

kernel_name = "dist_ag_xy_y_m1024_n512"

def setup_inputs():
    return {"x": np.random.randn(2048, 512).astype(np.float32)}

def reference(x: np.ndarray) -> np.ndarray:
    return x
```

```python
import jax
import jax.numpy as jnp
from jax import lax
from jax.experimental import pallas as pl
from jax.experimental.pallas import tpu as pltpu


def pallas_dist_ag_xy_y_m1024_n512_kernel(x: jax.Array):
    m, n = x.shape

    def body(x_ref, out_ref, send_buf, recv_buf, send_sem, recv_sem):
        my_x = lax.axis_index("x")
        my_y = lax.axis_index("y")
        send_buf[...] = x_ref[...].astype(jnp.bfloat16)
        rdma = pltpu.make_async_remote_copy(
            src_ref=send_buf, dst_ref=recv_buf, send_sem=send_sem, recv_sem=recv_sem,
            device_id=(my_x, 1 - my_y), device_id_type=pl.DeviceIdType.MESH)
        rdma.start()
        out_ref[pl.ds(pl.multiple_of(my_y * m, m), m), :] = x_ref[...]
        rdma.wait()
        out_ref[pl.ds(pl.multiple_of((1 - my_y) * m, m), m), :] = recv_buf[...].astype(jnp.float32)

    return pl.pallas_call(
        body,
        out_shape=jax.ShapeDtypeStruct((2 * m, n), x.dtype),
        in_specs=[pl.BlockSpec(memory_space=pltpu.VMEM)],
        out_specs=pl.BlockSpec(memory_space=pltpu.VMEM),
        scratch_shapes=[
            pltpu.VMEM((m, n), jnp.bfloat16),
            pltpu.VMEM((m, n), jnp.bfloat16),
            pltpu.SemaphoreType.DMA,
            pltpu.SemaphoreType.DMA,
        ],
    )(x)
```

```python
import jax
import jax.numpy as jnp
from jax import lax
from jax.experimental import pallas as pl
from jax.experimental.pallas import tpu as pltpu

_MESH = pl.DeviceIdType.MESH
_ROWS = 16
_LOAD_BLOCKS = (1, 3, 6, 19)
_EARLY_LOADS = 2
_N_BLOCKS = sum(_LOAD_BLOCKS)
_N_PIECES = 2 * _N_BLOCKS
_FILL_AFTER = 16


def pallas_dist_ag_xy_y_m1024_n512_kernel(x: jax.Array):
    m, n = x.shape
    w = n // 2
    s = _N_BLOCKS * _ROWS
    direct = m - 2 * s - _ROWS
    assert direct > 0 and direct % _ROWS == 0 and w % 128 == 0

    def rows(start, size):
        return pl.ds(pl.multiple_of(start, _ROWS), size)

    def body(x_hbm, out, xf, head_buf, load_sems, y_send, y_recv, x_send, x_recv, relay):
        my_x = lax.axis_index("x")
        my_y = lax.axis_index("y")
        y_nb = (my_x, 1 - my_y)
        x_nb = (1 - my_x, my_y)
        mine = my_y * m
        other = (1 - my_y) * m
        head_i, direct_i = _N_PIECES, _N_PIECES + 1

        def head_cols(xx):
            return pl.ds(pl.multiple_of(xx * w, w), w)

        def piece(i, base, xx):
            if i == head_i:
                return out.at[rows(base + 2 * s, _ROWS), head_cols(xx)]
            if i == direct_i:
                return out.at[rows(base + 2 * s + _ROWS, direct)]
            start = base + xx * s + (i // 2) * _ROWS
            return out.at[rows(start, _ROWS), pl.ds((i % 2) * w, w)]

        def y_copy(i, base):
            ref = piece(i, base, my_x)
            return pltpu.make_async_remote_copy(
                ref, ref, y_send.at[i], y_recv.at[i], device_id=y_nb, device_id_type=_MESH
            )

        def x_copy(i, xx):
            ref = piece(i, other, xx)
            return pltpu.make_async_remote_copy(
                ref, ref, x_send.at[i], x_recv.at[i], device_id=x_nb, device_id_type=_MESH
            )

        def load(start, size, sem):
            return pltpu.make_async_copy(
                x_hbm.at[rows(start, size)], xf.at[rows(start, size)], load_sems.at[sem]
            )

        def cast_own(start, size):
            out[rows(mine + start, size), :] = xf[rows(start, size), :].astype(out.dtype)

        loads, block = {}, 0
        for g, count in enumerate(_LOAD_BLOCKS):
            loads[block] = load(my_x * s + block * _ROWS, count * _ROWS, g)
            block += count
        tail_load = load(2 * s, m - 2 * s, len(_LOAD_BLOCKS))
        fill_load = load((1 - my_x) * s, s, len(_LOAD_BLOCKS) + 1)
        all_loads = [*loads.values(), tail_load, fill_load]

        def start_late_loads():
            for cp in all_loads[_EARLY_LOADS:]:
                cp.start()

        head = pltpu.make_async_remote_copy(
            x_hbm.at[rows(2 * s, _ROWS), head_cols(my_x)],
            head_buf,
            y_send.at[head_i],
            y_recv.at[head_i],
            device_id=y_nb,
            device_id_type=_MESH,
        )

        for cp in all_loads[:_EARLY_LOADS]:
            cp.start()

        barrier = pltpu.get_barrier_semaphore()
        pl.semaphore_signal(barrier, 1, device_id=y_nb, device_id_type=_MESH)

        @pl.when(my_y == 0)
        def _():
            pl.semaphore_signal(barrier, 1, device_id=x_nb, device_id_type=_MESH)
            start_late_loads()
            pl.semaphore_wait(barrier, 2)
            head.start()
            pl.semaphore_signal(relay, 1, device_id=x_nb, device_id_type=_MESH)

        @pl.when(my_y == 1)
        def _():
            pl.semaphore_wait(barrier, 1)
            head.start()

        for b in range(_N_BLOCKS):
            if b in loads:
                loads[b].wait()
            cast_own(my_x * s + b * _ROWS, _ROWS)
            y_copy(2 * b, mine).start()
            y_copy(2 * b + 1, mine).start()
            if b == 0:
                pl.when(my_y == 1)(start_late_loads)
        tail_load.wait()
        cast_own(2 * s, m - 2 * s)
        y_copy(direct_i, mine).start()

        pl.semaphore_wait(relay, 1)

        @pl.when(my_y == 0)
        def _():
            pl.semaphore_signal(relay, 1, device_id=y_nb, device_id_type=_MESH)

        head.wait_recv()
        head_val = head_buf[...].astype(out.dtype)
        for xx in range(2):

            @pl.when(my_x == xx)
            def _(xx=xx):
                out[rows(other + 2 * s, _ROWS), pl.ds(xx * w, w)] = head_val

        x_copy(head_i, my_x).start()
        for i in range(_N_PIECES):
            y_copy(i, other).wait_recv()
            x_copy(i, my_x).start()
            if i == _FILL_AFTER:
                fill_load.wait()
                cast_own((1 - my_x) * s, s)

        last = _N_PIECES - 1
        head.wait_send()
        for i in range(_N_PIECES):
            y_copy(i, mine).wait_send()
        for i in (head_i, *range(last)):
            x_copy(i, my_x).wait_send()
        for i in (head_i, *range(last)):
            x_copy(i, 1 - my_x).wait_recv()
        x_copy(last, my_x).wait_send()
        x_copy(last, 1 - my_x).wait_recv()
        y_copy(direct_i, mine).wait_send()
        y_copy(direct_i, other).wait_recv()

    return pl.pallas_call(
        body,
        out_shape=pltpu.VMEM((2 * m, n), jnp.bfloat16),
        in_specs=[pl.BlockSpec(memory_space=pltpu.HBM)],
        out_specs=pl.BlockSpec(memory_space=pltpu.VMEM),
        scratch_shapes=[
            pltpu.VMEM((m, n), x.dtype),
            pltpu.VMEM((_ROWS, w), x.dtype),
            pltpu.SemaphoreType.DMA((len(_LOAD_BLOCKS) + 2,)),
            pltpu.SemaphoreType.DMA((_N_PIECES + 2,)),
            pltpu.SemaphoreType.DMA((_N_PIECES + 2,)),
            pltpu.SemaphoreType.DMA((_N_PIECES + 1,)),
            pltpu.SemaphoreType.DMA((_N_PIECES + 1,)),
            pltpu.SemaphoreType.REGULAR,
        ],
        compiler_params=pltpu.CompilerParams(
            collective_id=0, disable_semaphore_checks=True
        ),
    )(x)
```
